```python
import numpy as np

kernel_name = "dist_moe_cap_ep_n512_d256_e4_h512"

def setup_inputs():
    x = np.random.randn(512, 256).astype(np.float32)
    router_W = np.random.randn(256, 16).astype(np.float32) * 0.1
    scores64 = x.astype(np.float64) @ router_W.astype(np.float64)
    route_idx = np.argsort(-scores64, axis=-1)[:, :1].astype(np.int32)
    expert_W = np.random.randn(16, 256, 512).astype(np.float32) * 0.02
    return {"x": x, "router_W": router_W, "route_idx": route_idx, "expert_W": expert_W}

def reference(x, router_W, route_idx, expert_W):
    counts = np.zeros(16, dtype=np.int64)
    out = np.zeros((512, 512), dtype=np.float32)
    for i in range(512):
        e = int(route_idx[i, 0])
        if counts[e] < 25:
            out[i] = x[i] @ expert_W[e]
            counts[e] += 1
    return out
```

```python
import contextlib
import functools
import re

import jax
import jax.numpy as jnp
from jax import lax
from jax.experimental import pallas as pl
from jax.experimental.pallas import tpu as pltpu

N_TOK, D_IN, D_OUT = 512, 256, 512
N_EXP, E_LOC, CAP, N_DEV = 16, 4, 25, 4
SLOTS = 32
MESH = pl.DeviceIdType.MESH
f32, bf16, i32, u32 = jnp.float32, jnp.bfloat16, jnp.int32, jnp.uint32


def iota(shape, dim):
    return lax.broadcasted_iota(i32, shape, dim)


def to_int(v):
    return pltpu.bitcast(v + 2.0**23, i32) & 0xFFFF


CH8 = tuple((e, c, 2) for e in range(4) for c in (0, 2))
CH9 = CH8[:-1] + ((3, 2, 1), (3, 3, 1))
CH10 = CH8[:-2] + ((3, 0, 1), (3, 1, 1), (3, 2, 1), (3, 3, 1))
CH11 = CH8[:-3] + ((2, 2, 1), (2, 3, 1), (3, 0, 1), (3, 1, 1), (3, 2, 1), (3, 3, 1))


def make(scopes=False, far=CH10, sw=(1, 2, 3, 4), a_order=None, prog=None, go_at=2, strided=False,
         sent_at=3, whole=1, gmode="when", late_b=None, **cp):
    def scope(name):
        on = scopes is True or (isinstance(scopes, str) and re.fullmatch(scopes, name))
        return jax.named_scope(name) if on else contextlib.nullcontext()

    near = CH8
    common = sum(a == b for a, b in zip(near, far))
    NCH = len(far)
    hw = [j for j in range(NCH) if j not in sw]
    late_b = hw if late_b is None else late_b
    cp.setdefault("disable_bounds_checks", True)
    cp.setdefault("disable_semaphore_checks", True)
    prog = prog or "G1 M0 M1 G2 M2 G3 " + " ".join(f"M{j}" for j in range(3, common))

    def running_count(idx_ref, e, b):
        own = jnp.zeros(e.shape, f32)
        before = jnp.zeros(e.shape, f32)
        for k in range(4):
            hit = (jnp.broadcast_to(idx_ref[pl.ds(k, 1), :], e.shape) & (N_EXP - 1)) == e
            own = jnp.where(hit & (b == k), 1.0, own)
            if k < 3:
                before = before + jnp.where(hit & (b > k), 1.0, 0.0)
        tri = jnp.where(iota((128, 128), 0) <= iota((128, 128), 1), 1.0, 0.0).astype(bf16)
        ones = jnp.ones((128, 128), bf16)
        return (jnp.dot(own.astype(bf16), tri, preferred_element_type=f32)
                + jnp.dot(before.astype(bf16), ones, preferred_element_type=f32))

    def slot_hits(cum, e):
        s = iota((SLOTS, 128), 0).astype(f32)
        acc = None
        for b in range(4):
            row = jnp.broadcast_to(cum[4 * e + b: 4 * e + b + 1, :], (SLOTS, 128))
            hit = jnp.where(row <= s, 1.0, 0.0)
            acc = hit if acc is None else acc + hit
        return acc

    def slot_tokens(cum, e):
        hits = slot_hits(cum, e)
        return to_int(jnp.broadcast_to(jnp.sum(hits, axis=1, keepdims=True), hits.shape))

    def body(x_hbm, idx_hbm, w_hbm, o_ref, idx_v, tok_v, xs, ws, ybuf, tab_v, tab_s,
             sem_in, sem_tab, sem_go, ssem, rsem):
        c_idx = pltpu.make_async_copy(idx_hbm, idx_v, sem_in.at[NCH + E_LOC])
        c_tab = pltpu.make_async_copy(tab_v, tab_s, sem_tab)

        def w_copy(j, chunk):
            e, c, n = chunk
            if e < whole:
                c, n = 0, 4
            cols = pl.ds(128 * c, 128 * n)
            return pltpu.make_async_copy(w_hbm.at[e, :, cols], ws.at[e, :, cols], sem_in.at[j])

        def has_copy(chunk):
            return chunk[0] >= whole or chunk[1] == 0

        c_idx.start()
        for j in range(common):
            if has_copy(near[j]):
                w_copy(j, near[j]).start(priority=1)

        me = lax.axis_index("i")
        right, left = (me + 1) & 3, (me + 3) & 3
        odd = (me & 1) == 1
        first = jnp.where(me == 3, right, left)
        second = (first + 2) & 3
        barrier = pltpu.get_barrier_semaphore()

        def remote(src, j, chunk, target, k):
            rows = ybuf.at[src, j, pl.ds(0, CAP if chunk[2] == 2 else (CAP + 1) // 2)]
            return pltpu.make_async_remote_copy(rows, rows, ssem.at[k * NCH + j], rsem.at[src * NCH + j],
                                                device_id=(target,), device_id_type=MESH)

        def scatter(src, j, chunk):
            e, c, n = chunk
            for s in range(CAP):
                off = tab_s[0, 128 * src + SLOTS * e + s] + 8 * c
                if n == 2:
                    v = ybuf[src, j, pl.ds(s, 1), :]
                    if strided:
                        v = jnp.broadcast_to(v, (8, 128))
                        v = (v << jnp.where(iota((8, 128), 0) == 0, 16, 0).astype(u32)) & jnp.uint32(0xFFFF0000)
                        o_ref[pl.ds(off, 2, stride=8), :] = pltpu.bitcast(v, f32)[:2]
                    else:
                        o_ref[pl.ds(off, 1), :] = pltpu.bitcast(v << 16, f32)
                        o_ref[pl.ds(off + 8, 1), :] = pltpu.bitcast(v & jnp.uint32(0xFFFF0000), f32)
                else:
                    v = ybuf[src, j, pl.ds(s // 2, 1), :]
                    v = v & jnp.uint32(0xFFFF0000) if s % 2 else v << 16
                    o_ref[pl.ds(off, 1), :] = pltpu.bitcast(v, f32)

        def make_table():
            r = iota((4 * N_EXP, 128), 0)
            cum_all = running_count(idx_v, r >> 2, r & 3)
            hits = jnp.concatenate([slot_hits(cum_all, g) for g in range(N_EXP)], axis=0).astype(bf16)
            tk = lax.dot_general(jnp.ones((16, 128), bf16), hits, (((1,), (1,)), ((), ())),
                                 preferred_element_type=f32)[:8]
            over = (iota(tk.shape, 1) & (SLOTS - 1)) >= CAP
            drop = jnp.min(jnp.where(over, tk, N_TOK - 1.0), axis=1, keepdims=True)
            t = to_int(jnp.where(tk < N_TOK, tk, drop))
            tab_v[...] = (((t >> 3) << 5) + (t & 7))[:1]
            c_tab.start()

        @pl.when(me != 2)
        def _():
            for nbr in (right, left):
                pl.semaphore_signal(barrier, inc=1, device_id=(nbr,), device_id_type=MESH)
            for j in range(common, len(near)):
                w_copy(j, near[j]).start(priority=1)

        @pl.when(me == 0)
        def _():
            pl.semaphore_signal(barrier, inc=1, device_id=(2,), device_id_type=MESH)

        o_ref[...] = jnp.zeros(o_ref.shape, f32)

        @pl.when(me == 2)
        def _():
            for j in range(common, len(far)):
                w_copy(j, far[j]).start(priority=1)
            pl.semaphore_wait(barrier, 3)
            for nbr in (1, 3):
                pl.semaphore_signal(sem_go, inc=1, device_id=(nbr,), device_id_type=MESH)

        def gather(e, tok):
            for s in range(CAP):
                t = tok[s, 0]
                pltpu.make_async_copy(x_hbm.at[t >> 3, :, t & 7], xs.at[e, :, s], sem_in.at[NCH + e]).start()

        r = iota((4 * E_LOC, 128), 0)
        e_of, b_of = E_LOC * me + (r >> 2), r & 3
        with scope("idx"):
            c_idx.wait()
        with scope("G0"):
            cum = running_count(idx_v, e_of, b_of)
            toks = [slot_tokens(cum, e) for e in range(E_LOC)]
            for e in range(E_LOC):
                tok_v[e] = toks[e]
            gather(0, toks[0] & (N_TOK - 1))

        def produce(j, chunk, rows_ready):
            e, c, n = chunk
            with scope(f"wait{j}"):
                if j == 0:
                    w_copy(j, chunk).wait()
                if e not in rows_ready:
                    rows_ready.add(e)
                    rows = xs.at[e, :, pl.ds(0, CAP)]
                    pltpu.make_async_copy(rows, rows, sem_in.at[NCH + e]).wait()
                xe = jnp.concatenate([xs[e, 0], xs[e, 1]], axis=1).astype(bf16)
                valid = (tok_v[e] < N_TOK) & (iota((SLOTS, 128), 0) < CAP)
                if j > 0 and has_copy(chunk):
                    w_copy(j, chunk).wait()
            y = jnp.dot(xe, ws[e, :, pl.ds(128 * c, 128 * n)].astype(bf16), preferred_element_type=f32)
            if n == 2:
                lo = jnp.where(valid, y[:, :128], 0.0)
                hi = jnp.where(valid, y[:, 128:], 0.0)
                bits = [pltpu.bitcast(v.astype(bf16).astype(f32), u32) for v in (lo, hi)]
                ybuf[me, j] = (bits[0] >> 16) | bits[1]
            else:
                ybuf[me, j, pl.ds(0, SLOTS // 2)] = pltpu.bitcast(jnp.where(valid, y, 0.0).astype(bf16), u32)

        rows_ready = set()
        z_done = []

        def z_forward(k):
            with scope(f"Z{k}"):
                remote(2, k, far[k], 0, 0).wait_recv()
            remote(2, k, far[k], 0, 2).start()

        for op in prog.split():
            k = int(op[1:])
            if op[0] == "G":
                def g(*_):
                    gather(k, tok_v[k] & (N_TOK - 1))

                with scope(op):
                    if gmode == "when":
                        pl.when(me < N_DEV)(g)
                    else:
                        lax.fori_loop(0, jnp.where(me < N_DEV, 1, 0), g, None)
            elif op[0] == "F":
                z_done.append(k)
                pl.when(me == 3)(functools.partial(z_forward, k))
            elif op[0] == "M":
                j, chunk = k, near[k]
                produce(j, chunk, rows_ready)
                if j == 0:
                    pl.when(me == 0)(make_table)

                    pl.when(me == 0)(lambda: pl.semaphore_wait(barrier, 2))
                    pl.when(odd)(lambda: pl.semaphore_wait(barrier, 1))
                remote(me, j, chunk, jnp.where(me == 2, 0, first) if j in hw else first, 0).start()
                if j < go_at:
                    @pl.when(jnp.logical_not(odd))
                    def _():
                        remote(me, j, chunk, second, 1).start()
                else:
                    if j == go_at:
                        @pl.when(odd)
                        def _():
                            pl.semaphore_wait(sem_go, 1)
                            for i in range(go_at):
                                remote(me, i, near[i], second, 1).start()
                    remote(me, j, chunk, second, 1).start()
                if j in hw and j not in late_b:
                    @pl.when(me == 2)
                    def _():
                        remote(2, j, chunk, 1, 2).start()
            else:
                raise ValueError(op)

        @pl.when(me == 2)
        def _():
            ready = set(rows_ready)
            for j in range(common, NCH):
                produce(j, far[j], ready)
                remote(2, j, far[j], 0 if j in hw else 1, 0).start()
                remote(2, j, far[j], 3, 1).start()
            for j in late_b:
                remote(2, j, far[j], 1, 2).start()

        @pl.when(me != 2)
        def _():
            ready = set(rows_ready)
            for j in range(common, len(near)):
                produce(j, near[j], ready)
                remote(me, j, near[j], first, 0).start()
                remote(me, j, near[j], second, 1).start()

        @pl.when(me == 3)
        def _():
            for j in sw:
                if j not in z_done:
                    z_forward(j)

        @pl.when(odd)
        def _():
            for j, chunk in enumerate(near):
                remote(0, j, chunk, 0, 0).wait_recv()

                @pl.when((me >> 1) == (j & 1))
                def _():
                    remote(0, j, chunk, 2, 3).start()

        pl.when(me != 0)(make_table)
        c_tab.wait()

        def step(n, c):
            src = jnp.where(n == 0, me, jnp.where(me == 2, (2 * n - 1) % 5,
                                                  jnp.where(n == 1, 0, jnp.where((n == 2) == (me == 1), 4 - me, 2))))
            seen = (n == 0) | ((src == 0) & (me != 2))

            @pl.when(src == 2)
            def _():
                for j, chunk in enumerate(far):
                    @pl.when((me == 1) if j in sw else (me != 2))
                    def _():
                        remote(2, j, chunk, 0, 0).wait_recv()
                    scatter(2, j, chunk)

            @pl.when(src != 2)
            def _():
                for j, chunk in enumerate(near):
                    @pl.when(jnp.logical_not(seen))
                    def _():
                        remote(src, j, chunk, 0, 0).wait_recv()
                    scatter(src, j, chunk)
            return c

        lax.fori_loop(0, jnp.where(me == 0, 1, N_DEV), step, 0)

        @pl.when(me != 2)
        def _():
            for j, chunk in enumerate(near):
                remote(me, j, chunk, first, 0).wait_send()
                remote(me, j, chunk, second, 1).wait_send()

        @pl.when(me == 2)
        def _():
            for j, chunk in enumerate(far):
                for k in range(3 if j in hw else 2):
                    remote(2, j, chunk, 1, k).wait_send()

        @pl.when(me == 3)
        def _():
            for j in sw:
                remote(2, j, far[j], 0, 2).wait_send()

        @pl.when(odd)
        def _():
            for j, chunk in enumerate(near):
                @pl.when((me >> 1) == (j & 1))
                def _():
                    remote(0, j, chunk, 2, 3).wait_send()

        @pl.when(me == 0)
        def _():
            order = [(t[0] if t[0] == "S" else int(t[0]), int(t[1:])) for t in a_order.split()]
            assert sorted(t for t in order if t[0] != "S") == [(s, j) for s in (1, 2, 3) for j in range(len(far if s == 2 else near))]
            pend = []
            for n, (src, j) in enumerate(order):
                if src == "S":
                    with scope("Asent"):
                        for _ in range(j):
                            pend.pop(0).wait_send()
                    continue
                chunk = (far if src == 2 else near)[j]
                with scope(f"A{src}_{j}"):
                    remote(src, j, chunk, 0, 0).wait_recv()
                if src != 2:
                    pend.append(remote(src, j, chunk, 4 - src, 2 + src // 2))
                    pend[-1].start()
                scatter(src, j, chunk)
            assert not pend

    def kernel(x, router_W, route_idx, expert_W):
        del router_W
        hbm = pl.BlockSpec(memory_space=pltpu.HBM)
        out = pl.pallas_call(
            body,
            out_shape=jax.ShapeDtypeStruct((N_TOK * D_OUT // 128, 128), f32),
            in_specs=[hbm, hbm, hbm],
            out_specs=pl.BlockSpec(memory_space=pltpu.VMEM),
            scratch_shapes=[
                pltpu.VMEM((4, 128), i32),
                pltpu.VMEM((E_LOC, SLOTS, 128), i32),
                pltpu.VMEM((E_LOC, 2, SLOTS, 128), f32),
                pltpu.VMEM((E_LOC, D_IN, D_OUT), f32),
                pltpu.VMEM((N_DEV, NCH, SLOTS, 128), u32),
                pltpu.VMEM((1, N_EXP * SLOTS), i32),
                pltpu.SMEM((1, N_EXP * SLOTS), i32),
                pltpu.SemaphoreType.DMA((NCH + E_LOC + 1,)),
                pltpu.SemaphoreType.DMA,
                pltpu.SemaphoreType.REGULAR,
                pltpu.SemaphoreType.DMA((4 * NCH,)),
                pltpu.SemaphoreType.DMA((N_DEV * NCH,)),
            ],
            compiler_params=pltpu.CompilerParams(collective_id=0, **cp),
        )(x.reshape(64, 8, 2, 128).transpose(0, 2, 1, 3), route_idx.reshape(4, 128), expert_W)
        return out.reshape(64, 4, 8, 128).transpose(0, 2, 1, 3).reshape(N_TOK, D_OUT)

    return kernel


o10 = "10 30 11 31 12 32 13 33 20 34 14 35 15 36 16 37 17 21 S10 25 22 26 S4 23 27 S2 28 24 29"
pallas_dist_moe_cap_ep_n512_d256_e4_h512_kernel = make(a_order=o10)
```

```python
import functools

import jax
import jax.numpy as jnp
from jax import lax
from jax.experimental import pallas as pl
from jax.experimental.pallas import tpu as pltpu

N_TOK, D_IN, D_OUT = 512, 256, 512
N_EXP, CAP, N_DEV = 16, 25, 4
E_LOC = N_EXP // N_DEV
SLOTS = 32
f32, bf16, i32, u32 = jnp.float32, jnp.bfloat16, jnp.int32, jnp.uint32

NEAR = tuple((e, c, 2) for e in range(E_LOC) for c in (0, 1))
FAR = NEAR[:-2] + tuple((E_LOC - 1, c, 1) for c in range(4))
N_SHARED = len(NEAR) - 2


def msg_rows(chunk):
    return CAP if chunk[2] == 2 else CAP // 2 + chunk[1] % 2


FAR_PARTS = (
    (0, 0, 0, CAP, False), (1, 0, 0, CAP, True), (2, 0, 0, CAP, True), (3, 0, 0, CAP, True),
    (4, 0, 0, 6, False), (4, 1, 6, CAP - 6, True), (5, 0, 0, CAP, False),
) + tuple((j, 0, 0, msg_rows(FAR[j]), False) for j in range(N_SHARED, len(FAR)))

ROOT_ORDER = (
    (1, 0), (3, 0), (1, 1), (3, 1), (1, 2), (3, 2), (1, 3), (3, 3), (2, 0), (3, 4), (1, 4),
    (3, 5), (1, 5), (3, 6), (1, 6), (3, 7), (1, 7), (2, 1), (2, 4), (None, 10), (2, 6), (2, 2),
    (2, 7), (None, 4), (2, 3), (2, 8), (None, 2), (2, 9), (2, 5), (2, 10),
)


def iota(shape, dim):
    return lax.broadcasted_iota(i32, shape, dim)


def to_int(v):
    return pltpu.bitcast(v + 2.0**23, i32) & 0xFFFF


def running_count(idx_ref, expert, block):
    own = jnp.zeros(expert.shape, f32)
    before = jnp.zeros(expert.shape, f32)
    for k in range(N_TOK // 128):
        routed = jnp.broadcast_to(idx_ref[pl.ds(k, 1), :], expert.shape) & (N_EXP - 1)
        hit = routed == expert
        own = jnp.where(hit & (block == k), 1.0, own)
        if k < N_TOK // 128 - 1:
            before = before + jnp.where(hit & (block > k), 1.0, 0.0)
    upper = jnp.where(iota((128, 128), 0) <= iota((128, 128), 1), 1.0, 0.0).astype(bf16)
    ones = jnp.ones((128, 128), bf16)
    return (jnp.dot(own.astype(bf16), upper, preferred_element_type=f32)
            + jnp.dot(before.astype(bf16), ones, preferred_element_type=f32))


def slot_hits(count):
    slot = iota((SLOTS, 128), 0).astype(f32)
    hits = [jnp.where(jnp.broadcast_to(count[b:b + 1], slot.shape) <= slot, 1.0, 0.0)
            for b in range(N_TOK // 128)]
    return functools.reduce(jnp.add, hits)


def slot_tokens(count):
    hits = slot_hits(count)
    return to_int(jnp.broadcast_to(jnp.sum(hits, axis=1, keepdims=True), hits.shape))


def moe_kernel(x_hbm, idx_hbm, w_hbm, o_ref, idx_v, count_v, tok_v, xs, ws, ybuf, dest_v, dest_s,
               in_sems, dest_sem, go_sem, send_sems, recv_sems):
    n_chunks = len(FAR)
    idx_copy = pltpu.make_async_copy(idx_hbm, idx_v, in_sems.at[n_chunks + E_LOC])
    dest_copy = pltpu.make_async_copy(dest_v, dest_s, dest_sem)

    def w_copy(j, chunk):
        e, c, n = chunk
        at = (e, slice(None), slice(None), c) if n == 2 else (e, slice(None), c // 2, c % 2)
        return pltpu.make_async_copy(w_hbm.at[at], ws.at[at], in_sems.at[j])

    idx_copy.start()
    for j in range(N_SHARED):
        w_copy(j, NEAR[j]).start(priority=1)

    me = lax.axis_index("i")
    right, left = (me + 1) & 3, (me + 3) & 3
    odd = (me & 1) == 1
    first = jnp.where(me == 3, right, left)
    second = (first + 2) & 3
    barrier = pltpu.get_barrier_semaphore()

    def signal(sem, chip):
        pl.semaphore_signal(sem, inc=1, device_id=(chip,), device_id_type=pl.DeviceIdType.MESH)

    def remote(src, j, row, rows, chip, use, part):
        msg = ybuf.at[src, j, pl.ds(row, rows)]
        return pltpu.make_async_remote_copy(
            msg, msg,
            send_sems.at[(2 * use + part) * n_chunks + j],
            recv_sems.at[(src + 2 * part) * n_chunks + j],
            device_id=(chip,), device_id_type=pl.DeviceIdType.MESH)

    def chunk_msg(src, j, chunk, chip=0, use=0):
        return remote(src, j, 0, msg_rows(chunk), chip, use, 0)

    def part_msg(far_part, chip=0, use=0):
        j, part, row, rows, _ = far_part
        return remote(2, j, row, rows, chip, use, part)

    @pl.when(me != 2)
    def _():
        signal(barrier, right)
        signal(barrier, left)
        for j in range(N_SHARED, len(NEAR)):
            w_copy(j, NEAR[j]).start(priority=1)

    pl.when(me == 0)(lambda: signal(barrier, 2))

    o_ref[...] = jnp.zeros(o_ref.shape, f32)
    xs[:, :, pl.ds(SLOTS - 8, 8)] = jnp.zeros((E_LOC, 2, 8, 128), f32)

    @pl.when(me == 2)
    def _():
        for j in range(N_SHARED, n_chunks):
            w_copy(j, FAR[j]).start(priority=1)
        pl.semaphore_wait(barrier, 3)
        signal(go_sem, 1)
        signal(go_sem, 3)

    pl.when(odd)(lambda: pl.semaphore_wait(barrier, 1))

    def fetch_rows(e, tok):
        tok = tok & (N_TOK - 1)
        for s in range(CAP):
            t = tok[s, 0]
            pltpu.make_async_copy(
                x_hbm.at[t >> 3, :, t & 7], xs.at[e, :, s], in_sems.at[n_chunks + e]).start()

    def produce(j, chunk, spare=0.0):
        e, c, n = chunk
        if j == 0:
            w_copy(j, chunk).wait()
        if c == 0:
            rows = xs.at[e, :, pl.ds(0, CAP)]
            pltpu.make_async_copy(rows, rows, in_sems.at[n_chunks + e]).wait()
        xe = jnp.concatenate([xs[e, 0], xs[e, 1]], axis=1).astype(bf16)
        filled = (tok_v[e] < N_TOK) & (iota((SLOTS, 128), 0) < CAP)
        if j > 0:
            w_copy(j, chunk).wait()
        w = [ws[e, :, t // 2, t % 2].reshape(D_IN, 128).astype(bf16) for t in range(c, c + 2 * n, 2)]
        if n == 2:
            y = [jnp.where(filled, jnp.dot(xe, t, preferred_element_type=f32), 0.0) for t in w]
            lo, hi = [pltpu.bitcast(v.astype(bf16).astype(f32), u32) for v in y]
            ybuf[me, j] = (lo >> 16) | hi
            return None
        for h in range(2):
            half = slice(16 * h, 16 * h + 16)
            y = jnp.dot(xe[half], w[0], preferred_element_type=f32)
            y = jnp.where(filled[half], y, spare if h else 0.0)
            ybuf[me, j, pl.ds(8 * h, 8)] = pltpu.bitcast(y.astype(bf16), u32)
        if c % 2:
            return 0.0
        return jnp.concatenate([jnp.zeros((8, 128), f32), pltpu.roll(y[8:], 1, 0)], axis=0)

    def send_far(j):
        mine = [p for p in FAR_PARTS if p[0] == j]
        for p in mine:
            if not p[4]:
                part_msg(p, 0, 2).start()
        for p in mine:
            part_msg(p, 3, 1).start()
        if all(p[4] for p in mine):
            chunk_msg(2, j, FAR[j], 1, 0).start()

    def send_near(j):
        chunk_msg(me, j, NEAR[j], first, 0).start()
        if j < 2:
            pl.when(me == 0)(chunk_msg(me, j, NEAR[j], second, 1).start)
            return
        if j == 2:
            @pl.when(odd)
            def _():
                pl.semaphore_wait(go_sem, 1)
                for i in range(j):
                    chunk_msg(me, i, NEAR[i], second, 1).start()
        chunk_msg(me, j, NEAR[j], second, 1).start()

    def find_destinations():
        r = iota((4 * N_EXP, 128), 0)
        count = running_count(idx_v, r >> 2, r & 3)
        hits = jnp.concatenate([slot_hits(count[4 * g:4 * g + 4]) for g in range(N_EXP)], axis=0)
        tok = lax.dot_general(jnp.ones((16, 128), bf16), hits.astype(bf16), (((1,), (1,)), ((), ())),
                              preferred_element_type=f32)[:8]
        over = (iota(tok.shape, 1) & (SLOTS - 1)) >= CAP
        dropped = jnp.min(jnp.where(over, tok, N_TOK - 1.0), axis=1, keepdims=True)
        t = to_int(jnp.where(tok < N_TOK, tok, dropped))
        dest_v[...] = (((t >> 3) << 5) + (t & 7))[:1]
        dest_copy.start()

    def scatter(src, j, chunk, row=0, rows=None):
        e, c, n = chunk
        for r in range(row, row + (rows or msg_rows(chunk))):
            if n == 2:
                halves = ((r, c), (r, c + 2))
            else:
                halves = ((2 * r, c), (2 * r + 1, c) if 2 * r + 1 < CAP else (2 * r, c - 1))
            word = ybuf[src, j, pl.ds(r, 1), :]
            for bits, (slot, tile) in zip((word << 16, word & jnp.uint32(0xFFFF0000)), halves):
                at = dest_s[0, SLOTS * (E_LOC * src + e) + slot] + 8 * tile
                o_ref[pl.ds(at, 1), :] = pltpu.bitcast(bits, f32)

    r = iota((4 * E_LOC, 128), 0)
    expert, block = E_LOC * me + (r >> 2), r & 3
    idx_copy.wait()
    count = running_count(idx_v, expert, block)
    count_v[...] = count
    tok = slot_tokens(count[:4])
    tok_v[0] = tok
    fetch_rows(0, tok)
    for e in range(1, E_LOC):
        tok_v[e] = slot_tokens(count_v[pl.ds(4 * e, 4), :])
    fetch_rows(1, tok_v[1])

    for j in range(N_SHARED):
        produce(j, NEAR[j])
        if j == 0:
            @pl.when(me == 0)
            def _():
                find_destinations()
                pl.semaphore_wait(barrier, 2)
        pl.when(me != 2)(functools.partial(send_near, j))
        pl.when(me == 2)(functools.partial(send_far, j))
        if j in (1, 2):
            fetch_rows(j + 1, tok_v[j + 1])

    @pl.when(me == 2)
    def _():
        spare = 0.0
        for j in range(N_SHARED, n_chunks):
            spare = produce(j, FAR[j], spare)
            send_far(j)
        for j in sorted({p[0] for p in FAR_PARTS if not p[4]}):
            chunk_msg(2, j, FAR[j], 1, 0).start()

    @pl.when(me != 2)
    def _():
        for j in range(N_SHARED, len(NEAR)):
            produce(j, NEAR[j])
            send_near(j)

    @pl.when(me == 3)
    def _():
        for p in FAR_PARTS:
            if p[4]:
                part_msg(p).wait_recv()
                part_msg(p, 0, 2).start()

    @pl.when(odd)
    def _():
        for j, chunk in enumerate(NEAR):
            chunk_msg(0, j, chunk).wait_recv()
            pl.when((me >> 1) == (j & 1))(chunk_msg(0, j, chunk, 2, 3).start)

    pl.when(me != 0)(find_destinations)
    dest_copy.wait()

    def scatter_chip(n, carry):
        src = jnp.where(me == 2, (2 * n - 1) % 5,
                        jnp.where(n == 1, 0, jnp.where((n == 2) == (me == 1), 4 - me, 2)))
        src = jnp.where(n == 0, me, src)
        landed = (n == 0) | ((src == 0) & odd)

        @pl.when(src == 2)
        def _():
            for j, chunk in enumerate(FAR):
                pl.when(me == 1)(chunk_msg(2, j, chunk).wait_recv)
                for p in FAR_PARTS:
                    if p[0] == j and not p[4]:
                        pl.when(me == 3)(part_msg(p).wait_recv)
                scatter(2, j, chunk)

        @pl.when(src != 2)
        def _():
            for j, chunk in enumerate(NEAR):
                pl.when(jnp.logical_not(landed))(chunk_msg(src, j, chunk).wait_recv)
                scatter(src, j, chunk)

        return carry

    lax.fori_loop(0, jnp.where(me == 0, 1, N_DEV), scatter_chip, 0)

    @pl.when(me != 2)
    def _():
        for j, chunk in enumerate(NEAR):
            chunk_msg(me, j, chunk, first, 0).wait_send()
            chunk_msg(me, j, chunk, second, 1).wait_send()

    @pl.when(me == 2)
    def _():
        for j, chunk in enumerate(FAR):
            chunk_msg(2, j, chunk, 1, 0).wait_send()
        for p in FAR_PARTS:
            part_msg(p, 3, 1).wait_send()
            if not p[4]:
                part_msg(p, 0, 2).wait_send()

    @pl.when(me == 3)
    def _():
        for p in FAR_PARTS:
            if p[4]:
                part_msg(p, 0, 2).wait_send()

    @pl.when(odd)
    def _():
        for j, chunk in enumerate(NEAR):
            pl.when((me >> 1) == (j & 1))(chunk_msg(0, j, chunk, 2, 3).wait_send)

    @pl.when(me == 0)
    def _():
        forwarded = []
        for src, k in ROOT_ORDER:
            if src is None:
                for _ in range(k):
                    forwarded.pop(0).wait_send()
            elif src == 2:
                j, _, row, rows, _ = FAR_PARTS[k]
                part_msg(FAR_PARTS[k]).wait_recv()
                scatter(2, j, FAR[j], row, rows)
            else:
                chunk_msg(src, k, NEAR[k]).wait_recv()
                forwarded.append(chunk_msg(src, k, NEAR[k], 4 - src, 2 + src // 2))
                forwarded[-1].start()
                scatter(src, k, NEAR[k])
        assert not forwarded


def pallas_dist_moe_cap_ep_n512_d256_e4_h512_kernel(
    x: jax.Array,
    router_W: jax.Array,
    route_idx: jax.Array,
    expert_W: jax.Array,
):
    del router_W
    n_chunks = len(FAR)
    hbm = pl.BlockSpec(memory_space=pltpu.HBM)
    out = pl.pallas_call(
        moe_kernel,
        out_shape=jax.ShapeDtypeStruct((N_TOK * D_OUT // 128, 128), f32),
        in_specs=[hbm, hbm, hbm],
        out_specs=pl.BlockSpec(memory_space=pltpu.VMEM),
        scratch_shapes=[
            pltpu.VMEM((N_TOK // 128, 128), i32),
            pltpu.VMEM((4 * E_LOC, 128), f32),
            pltpu.VMEM((E_LOC, SLOTS, 128), i32),
            pltpu.VMEM((E_LOC, 2, SLOTS, 128), f32),
            pltpu.VMEM((E_LOC, D_IN // 8, 2, 2, 8, 128), f32),
            pltpu.VMEM((N_DEV, n_chunks, SLOTS, 128), u32),
            pltpu.VMEM((1, N_EXP * SLOTS), i32),
            pltpu.SMEM((1, N_EXP * SLOTS), i32),
            pltpu.SemaphoreType.DMA((n_chunks + E_LOC + 1,)),
            pltpu.SemaphoreType.DMA,
            pltpu.SemaphoreType.REGULAR,
            pltpu.SemaphoreType.DMA((8 * n_chunks,)),
            pltpu.SemaphoreType.DMA(((N_DEV + 1) * n_chunks,)),
        ],
        compiler_params=pltpu.CompilerParams(
            collective_id=0,
            disable_bounds_checks=True,
            disable_semaphore_checks=True,
            flags={"XLA_TPU_FORCE_LP_LLO_SCHEDULER": True},
        ),
    )(
        x.reshape(N_TOK // 8, 8, 2, 128).transpose(0, 2, 1, 3),
        route_idx.reshape(N_TOK // 128, 128),
        expert_W.reshape(E_LOC, D_IN // 8, 8, 2, 2, 128).transpose(0, 1, 3, 4, 2, 5),
    )
    return out.reshape(N_TOK // 8, 4, 8, 128).transpose(0, 2, 1, 3).reshape(N_TOK, D_OUT)
```

```python
import functools

import jax
import jax.numpy as jnp
from jax import lax
from jax.experimental import pallas as pl
from jax.experimental.pallas import tpu as pltpu

N_TOK, D_IN, D_OUT = 512, 256, 512
N_EXP, CAP, N_DEV = 16, 25, 4
E_LOC = N_EXP // N_DEV
SLOTS = 32
f32, bf16, i32, u32 = jnp.float32, jnp.bfloat16, jnp.int32, jnp.uint32

NEAR = tuple((e, c, 2) for e in range(E_LOC) for c in (0, 1))
FAR = NEAR[:-2] + tuple((E_LOC - 1, c, 1) for c in range(4))
N_SHARED = len(NEAR) - 2


def msg_rows(chunk):
    return CAP if chunk[2] == 2 else CAP // 2 + chunk[1] % 2


FAR_PARTS = (
    (0, 0, 0, CAP, False), (1, 0, 0, CAP, True), (2, 0, 0, CAP, True), (3, 0, 0, CAP, True),
    (4, 0, 0, 6, False), (4, 1, 6, CAP - 6, True), (5, 0, 0, CAP, False),
) + tuple((j, 0, 0, msg_rows(FAR[j]), False) for j in range(N_SHARED, len(FAR)))
LAST_FORWARDED = 1 + max(p[0] for p in FAR_PARTS if p[4])

ROOT_ORDER = (
    (1, 0), (3, 0), (1, 1), (3, 1), (1, 2), (3, 2), (1, 3), (3, 3), (2, 0), (3, 4), (1, 4),
    (3, 5), (1, 5), (3, 6), (1, 6), (3, 7), (1, 7), (2, 1), (2, 4), (None, 10), (2, 6), (2, 2),
    (2, 7), (2, 3), (None, 6), (2, 8), (2, 9), (2, 5), (2, 10),
)


def iota(shape, dim):
    return lax.broadcasted_iota(i32, shape, dim)


def to_int(v):
    return pltpu.bitcast(v + 2.0**23, i32) & 0xFFFF


def running_count(idx_ref, expert, block):
    own = jnp.zeros(expert.shape, f32)
    before = jnp.zeros(expert.shape, f32)
    for k in range(N_TOK // 128):
        routed = jnp.broadcast_to(idx_ref[pl.ds(k, 1), :], expert.shape) & (N_EXP - 1)
        hit = routed == expert
        own = jnp.where(hit & (block == k), 1.0, own)
        if k < N_TOK // 128 - 1:
            before = before + jnp.where(hit & (block > k), 1.0, 0.0)
    upper = jnp.where(iota((128, 128), 0) <= iota((128, 128), 1), 1.0, 0.0).astype(bf16)
    ones = jnp.ones((128, 128), bf16)
    return (jnp.dot(own.astype(bf16), upper, preferred_element_type=f32)
            + jnp.dot(before.astype(bf16), ones, preferred_element_type=f32))


def slot_hits(count):
    slot = iota((SLOTS, 128), 0).astype(f32)
    hits = [jnp.where(jnp.broadcast_to(count[b:b + 1], slot.shape) <= slot, 1.0, 0.0)
            for b in range(N_TOK // 128)]
    return functools.reduce(jnp.add, hits)


def slot_tokens(count):
    hits = slot_hits(count)
    return to_int(jnp.broadcast_to(jnp.sum(hits, axis=1, keepdims=True), hits.shape))


def moe_kernel(x_hbm, idx_hbm, w_hbm, o_ref, idx_v, count_v, tok_v, xs, ws, ybuf, dest_v, dest_s,
               in_sems, dest_sem, go_sem, send_sems, recv_sems):
    n_chunks = len(FAR)
    idx_copy = pltpu.make_async_copy(idx_hbm, idx_v, in_sems.at[n_chunks + E_LOC])
    dest_copy = pltpu.make_async_copy(dest_v, dest_s, dest_sem)

    def w_copy(j, chunk):
        e, c, n = chunk
        at = (e, slice(None), slice(None), c) if n == 2 else (e, slice(None), c // 2, c % 2)
        return pltpu.make_async_copy(w_hbm.at[at], ws.at[at], in_sems.at[j])

    idx_copy.start()
    for j in range(N_SHARED):
        w_copy(j, NEAR[j]).start(priority=1)

    me = lax.axis_index("i")
    right, left = (me + 1) & 3, (me + 3) & 3
    odd = (me & 1) == 1
    first = jnp.where(me == 3, right, left)
    second = (first + 2) & 3
    barrier = pltpu.get_barrier_semaphore()

    def signal(sem, chip):
        pl.semaphore_signal(sem, inc=1, device_id=(chip,), device_id_type=pl.DeviceIdType.MESH)

    def remote(src, j, row, rows, chip, use, part):
        msg = ybuf.at[src, j, pl.ds(row, rows)]
        return pltpu.make_async_remote_copy(
            msg, msg,
            send_sems.at[(2 * use + part) * n_chunks + j],
            recv_sems.at[(src + 2 * part) * n_chunks + j],
            device_id=(chip,), device_id_type=pl.DeviceIdType.MESH)

    def chunk_msg(src, j, chunk, chip=0, use=0):
        return remote(src, j, 0, msg_rows(chunk), chip, use, 0)

    def part_msg(far_part, chip=0, use=0):
        j, part, row, rows, _ = far_part
        return remote(2, j, row, rows, chip, use, part)

    @pl.when(me != 2)
    def _():
        signal(barrier, right)
        signal(barrier, left)
        for j in range(N_SHARED, len(NEAR)):
            w_copy(j, NEAR[j]).start(priority=1)

    pl.when(me == 0)(lambda: signal(barrier, 2))

    o_ref[...] = jnp.zeros(o_ref.shape, f32)
    xs[:, :, pl.ds(SLOTS - 8, 8)] = jnp.zeros((E_LOC, 2, 8, 128), f32)

    @pl.when(me == 2)
    def _():
        for j in range(N_SHARED, n_chunks):
            w_copy(j, FAR[j]).start(priority=1)
        pl.semaphore_wait(barrier, 3)
        signal(go_sem, 1)
        signal(go_sem, 3)

    pl.when(odd)(lambda: pl.semaphore_wait(barrier, 1))

    def fetch_rows(e, tok):
        tok = tok & (N_TOK - 1)
        for s in range(CAP):
            t = tok[s, 0]
            pltpu.make_async_copy(
                x_hbm.at[t >> 3, :, t & 7], xs.at[e, :, s], in_sems.at[n_chunks + e]).start()

    def produce(j, chunk, spare=0.0):
        e, c, n = chunk
        if j == 0:
            w_copy(j, chunk).wait()
        if c == 0:
            rows = xs.at[e, :, pl.ds(0, CAP)]
            pltpu.make_async_copy(rows, rows, in_sems.at[n_chunks + e]).wait()
        xe = jnp.concatenate([xs[e, 0], xs[e, 1]], axis=1).astype(bf16)
        filled = (tok_v[e] < N_TOK) & (iota((SLOTS, 128), 0) < CAP)
        if j > 0:
            w_copy(j, chunk).wait()
        w = [ws[e, :, t // 2, t % 2].reshape(D_IN, 128).astype(bf16) for t in range(c, c + 2 * n, 2)]
        if n == 2:
            y = [jnp.where(filled, jnp.dot(xe, t, preferred_element_type=f32), 0.0) for t in w]
            lo, hi = [pltpu.bitcast(v.astype(bf16).astype(f32), u32) for v in y]
            ybuf[me, j] = (lo >> 16) | hi
            return None
        for h in range(2):
            half = slice(16 * h, 16 * h + 16)
            y = jnp.dot(xe[half], w[0], preferred_element_type=f32)
            y = jnp.where(filled[half], y, spare if h else 0.0)
            ybuf[me, j, pl.ds(8 * h, 8)] = pltpu.bitcast(y.astype(bf16), u32)
        if c % 2:
            return 0.0
        return jnp.concatenate([jnp.zeros((8, 128), f32), pltpu.roll(y[8:], 1, 0)], axis=0)

    def send_far(j):
        mine = [p for p in FAR_PARTS if p[0] == j]
        for p in mine:
            if not p[4]:
                part_msg(p, 0, 2).start()
        for p in mine:
            if p[4] or j >= LAST_FORWARDED:
                part_msg(p, 3, 1).start()
        if all(p[4] for p in mine):
            chunk_msg(2, j, FAR[j], 1, 0).start()

    def send_near(j):
        chunk_msg(me, j, NEAR[j], first, 0).start()
        if j < 2:
            pl.when(me == 0)(chunk_msg(me, j, NEAR[j], second, 1).start)
            return
        if j == 2:
            @pl.when(odd)
            def _():
                pl.semaphore_wait(go_sem, 1)
                for i in range(j):
                    chunk_msg(me, i, NEAR[i], second, 1).start()
        chunk_msg(me, j, NEAR[j], second, 1).start()

    def find_destinations():
        r = iota((4 * N_EXP, 128), 0)
        count = running_count(idx_v, r >> 2, r & 3)
        hits = jnp.concatenate([slot_hits(count[4 * g:4 * g + 4]) for g in range(N_EXP)], axis=0)
        tok = lax.dot_general(jnp.ones((16, 128), bf16), hits.astype(bf16), (((1,), (1,)), ((), ())),
                              preferred_element_type=f32)[:8]
        over = (iota(tok.shape, 1) & (SLOTS - 1)) >= CAP
        dropped = jnp.min(jnp.where(over, tok, N_TOK - 1.0), axis=1, keepdims=True)
        t = to_int(jnp.where(tok < N_TOK, tok, dropped))
        dest_v[...] = (((t >> 3) << 5) + (t & 7))[:1]
        dest_copy.start()

    def scatter(src, j, chunk, row=0, rows=None):
        e, c, n = chunk
        for r in range(row, row + (rows or msg_rows(chunk))):
            if n == 2:
                halves = ((r, c), (r, c + 2))
            else:
                halves = ((2 * r, c), (2 * r + 1, c) if 2 * r + 1 < CAP else (2 * r, c - 1))
            word = ybuf[src, j, pl.ds(r, 1), :]
            for bits, (slot, tile) in zip((word << 16, word & jnp.uint32(0xFFFF0000)), halves):
                at = dest_s[0, SLOTS * (E_LOC * src + e) + slot] + 8 * tile
                o_ref[pl.ds(at, 1), :] = pltpu.bitcast(bits, f32)

    r = iota((4 * E_LOC, 128), 0)
    expert, block = E_LOC * me + (r >> 2), r & 3
    idx_copy.wait()
    count = running_count(idx_v, expert, block)
    count_v[...] = count
    tok = slot_tokens(count[:4])
    tok_v[0] = tok
    fetch_rows(0, tok)
    for e in range(1, E_LOC):
        tok_v[e] = slot_tokens(count_v[pl.ds(4 * e, 4), :])
    fetch_rows(1, tok_v[1])

    for j in range(N_SHARED):
        produce(j, NEAR[j])
        if j == 0:
            @pl.when(me == 0)
            def _():
                find_destinations()
                pl.semaphore_wait(barrier, 2)
        pl.when(me != 2)(functools.partial(send_near, j))
        pl.when(me == 2)(functools.partial(send_far, j))
        if j in (1, 2):
            fetch_rows(j + 1, tok_v[j + 1])

    @pl.when(me == 2)
    def _():
        spare = 0.0
        for j in range(N_SHARED, n_chunks):
            spare = produce(j, FAR[j], spare)
            send_far(j)
        for p in FAR_PARTS:
            if not p[4] and p[0] < LAST_FORWARDED:
                part_msg(p, 3, 1).start()
        for j in sorted({p[0] for p in FAR_PARTS if not p[4]}):
            chunk_msg(2, j, FAR[j], 1, 0).start()

    @pl.when(me != 2)
    def _():
        for j in range(N_SHARED, len(NEAR)):
            produce(j, NEAR[j])
            send_near(j)

    @pl.when(me == 3)
    def _():
        for p in FAR_PARTS:
            if p[4]:
                part_msg(p).wait_recv()
                part_msg(p, 0, 2).start()

    @pl.when(odd)
    def _():
        for j, chunk in enumerate(NEAR):
            chunk_msg(0, j, chunk).wait_recv()
            pl.when((me >> 1) == (j & 1))(chunk_msg(0, j, chunk, 2, 3).start)

    pl.when(me != 0)(find_destinations)
    dest_copy.wait()

    def scatter_chip(n, carry):
        src = jnp.where(me == 2, (2 * n - 1) % 5,
                        jnp.where(n == 1, 0, jnp.where((n == 2) == (me == 1), 4 - me, 2)))
        src = jnp.where(n == 0, me, src)
        landed = (n == 0) | ((src == 0) & odd)

        @pl.when(src == 2)
        def _():
            for j, chunk in enumerate(FAR):
                pl.when(me == 1)(chunk_msg(2, j, chunk).wait_recv)
                for p in FAR_PARTS:
                    if p[0] == j and not p[4]:
                        pl.when(me == 3)(part_msg(p).wait_recv)
                scatter(2, j, chunk)

        @pl.when(src != 2)
        def _():
            for j, chunk in enumerate(NEAR):
                pl.when(jnp.logical_not(landed))(chunk_msg(src, j, chunk).wait_recv)
                scatter(src, j, chunk)

        return carry

    lax.fori_loop(0, jnp.where(me == 0, 1, N_DEV), scatter_chip, 0)

    @pl.when(me != 2)
    def _():
        for j, chunk in enumerate(NEAR):
            chunk_msg(me, j, chunk, first, 0).wait_send()
            chunk_msg(me, j, chunk, second, 1).wait_send()

    @pl.when(me == 2)
    def _():
        for j, chunk in enumerate(FAR):
            chunk_msg(2, j, chunk, 1, 0).wait_send()
        for p in FAR_PARTS:
            part_msg(p, 3, 1).wait_send()
            if not p[4]:
                part_msg(p, 0, 2).wait_send()

    @pl.when(me == 3)
    def _():
        for p in FAR_PARTS:
            if p[4]:
                part_msg(p, 0, 2).wait_send()

    @pl.when(odd)
    def _():
        for j, chunk in enumerate(NEAR):
            pl.when((me >> 1) == (j & 1))(chunk_msg(0, j, chunk, 2, 3).wait_send)

    @pl.when(me == 0)
    def _():
        forwarded = []
        for src, k in ROOT_ORDER:
            if src is None:
                for _ in range(k):
                    forwarded.pop(0).wait_send()
            elif src == 2:
                j, _, row, rows, _ = FAR_PARTS[k]
                part_msg(FAR_PARTS[k]).wait_recv()
                scatter(2, j, FAR[j], row, rows)
            else:
                chunk_msg(src, k, NEAR[k]).wait_recv()
                forwarded.append(chunk_msg(src, k, NEAR[k], 4 - src, 2 + src // 2))
                forwarded[-1].start()
                scatter(src, k, NEAR[k])
        assert not forwarded


def pallas_dist_moe_cap_ep_n512_d256_e4_h512_kernel(
    x: jax.Array,
    router_W: jax.Array,
    route_idx: jax.Array,
    expert_W: jax.Array,
):
    del router_W
    n_chunks = len(FAR)
    hbm = pl.BlockSpec(memory_space=pltpu.HBM)
    out = pl.pallas_call(
        moe_kernel,
        out_shape=jax.ShapeDtypeStruct((N_TOK * D_OUT // 128, 128), f32),
        in_specs=[hbm, hbm, hbm],
        out_specs=pl.BlockSpec(memory_space=pltpu.VMEM),
        scratch_shapes=[
            pltpu.VMEM((N_TOK // 128, 128), i32),
            pltpu.VMEM((4 * E_LOC, 128), f32),
            pltpu.VMEM((E_LOC, SLOTS, 128), i32),
            pltpu.VMEM((E_LOC, 2, SLOTS, 128), f32),
            pltpu.VMEM((E_LOC, D_IN // 8, 2, 2, 8, 128), f32),
            pltpu.VMEM((N_DEV, n_chunks, SLOTS, 128), u32),
            pltpu.VMEM((1, N_EXP * SLOTS), i32),
            pltpu.SMEM((1, N_EXP * SLOTS), i32),
            pltpu.SemaphoreType.DMA((n_chunks + E_LOC + 1,)),
            pltpu.SemaphoreType.DMA,
            pltpu.SemaphoreType.REGULAR,
            pltpu.SemaphoreType.DMA((8 * n_chunks,)),
            pltpu.SemaphoreType.DMA(((N_DEV + 1) * n_chunks,)),
        ],
        compiler_params=pltpu.CompilerParams(
            collective_id=0,
            disable_bounds_checks=True,
            disable_semaphore_checks=True,
            flags={"XLA_TPU_FORCE_LP_LLO_SCHEDULER": True},
        ),
    )(
        x.reshape(N_TOK // 8, 8, 2, 128).transpose(0, 2, 1, 3),
        route_idx.reshape(N_TOK // 128, 128),
        expert_W.reshape(E_LOC, D_IN // 8, 8, 2, 2, 128).transpose(0, 1, 3, 4, 2, 5),
    )
    return out.reshape(N_TOK // 8, 4, 8, 128).transpose(0, 2, 1, 3).reshape(N_TOK, D_OUT)
```

```python
import functools

import jax
import jax.numpy as jnp
from jax import lax
from jax.experimental import pallas as pl
from jax.experimental.pallas import tpu as pltpu

N_TOK, D_IN, D_OUT = 512, 256, 512
N_EXP, CAP, N_DEV = 16, 25, 4
E_LOC = N_EXP // N_DEV
SLOTS = 32
f32, bf16, i32, u32 = jnp.float32, jnp.bfloat16, jnp.int32, jnp.uint32

CHUNKS = (
    (0, 0, 2), (0, 1, 2), (1, 0, 2), (1, 1, 2), (2, 0, 2),
    (2, 1, 1), (2, 3, 1), (3, 0, 1), (3, 1, 1), (3, 2, 1), (3, 3, 1),
)
LEADING = (5, 7, 9)
N_CHUNKS = len(CHUNKS)


def msg_rows(j):
    return CAP if CHUNKS[j][2] == 2 else CAP // 2 + (j not in LEADING)


N_EARLY = 5
FAR_PARTS = (
    (0, 0, 0, CAP, False), (1, 0, 0, CAP, True), (2, 0, 0, CAP, True), (3, 0, 0, CAP, True),
    (4, 0, 0, 6, False), (4, 1, 6, CAP - 6, True),
) + tuple((j, 0, 0, msg_rows(j), False) for j in range(N_EARLY, N_CHUNKS))

ROOT_ORDER = (
    (0, 0), (0, 1), (0, 2), (0, 3), (1, 0), (3, 0), (1, 1), (3, 1), (1, 2), (3, 2),
    (0, 4), (0, 5), (1, 3), (3, 3), (0, 6), (0, 7), (0, 8), (0, 9), (0, 10), (None, 22),
    (3, 4), (2, 0), (1, 4), (3, 5), (3, 6), (1, 5), (3, 7), (1, 6), (3, 8), (1, 7),
    (3, 9), (1, 8), (3, 10), (1, 9), (1, 10), (2, 1), (2, 4), (None, 14), (2, 6), (2, 2),
    (None, 8), (2, 7), (2, 8), (2, 3), (2, 9), (2, 10), (2, 5), (2, 11),
)


def iota(shape, dim):
    return lax.broadcasted_iota(i32, shape, dim)


def to_int(v):
    return pltpu.bitcast(v + 2.0**23, i32) & 0xFFFF


def running_count(idx_ref, expert, block):
    own = jnp.zeros(expert.shape, f32)
    before = jnp.zeros(expert.shape, f32)
    for k in range(N_TOK // 128):
        routed = jnp.broadcast_to(idx_ref[pl.ds(k, 1), :], expert.shape) & (N_EXP - 1)
        hit = routed == expert
        own = jnp.where(hit & (block == k), 1.0, own)
        if k < N_TOK // 128 - 1:
            before = before + jnp.where(hit & (block > k), 1.0, 0.0)
    upper = jnp.where(iota((128, 128), 0) <= iota((128, 128), 1), 1.0, 0.0).astype(bf16)
    ones = jnp.ones((128, 128), bf16)
    return (jnp.dot(own.astype(bf16), upper, preferred_element_type=f32)
            + jnp.dot(before.astype(bf16), ones, preferred_element_type=f32))


def slot_hits(count):
    slot = iota((SLOTS, 128), 0).astype(f32)
    hits = [jnp.where(jnp.broadcast_to(count[b:b + 1], slot.shape) <= slot, 1.0, 0.0)
            for b in range(N_TOK // 128)]
    return functools.reduce(jnp.add, hits)


def slot_tokens(count):
    hits = slot_hits(count)
    return to_int(jnp.broadcast_to(jnp.sum(hits, axis=1, keepdims=True), hits.shape))


def moe_kernel(x_hbm, idx_hbm, w_hbm, o_ref, idx_v, count_v, tok_v, xs, ws, ybuf, dest_v, dest_s,
               in_sems, dest_sem, go_sem, send_sems, recv_sems):
    idx_copy = pltpu.make_async_copy(idx_hbm, idx_v, in_sems.at[N_CHUNKS + E_LOC])
    dest_copy = pltpu.make_async_copy(dest_v, dest_s, dest_sem)

    def w_copy(j):
        e, c, n = CHUNKS[j]
        at = (e, slice(None), slice(None), c) if n == 2 else (e, slice(None), c // 2, c % 2)
        return pltpu.make_async_copy(w_hbm.at[at], ws.at[at], in_sems.at[j])

    idx_copy.start()
    for j in range(N_CHUNKS):
        w_copy(j).start(priority=1)

    me = lax.axis_index("i")
    right, left = (me + 1) & 3, (me + 3) & 3
    odd = (me & 1) == 1
    first = jnp.where(me == 3, right, left)
    second = (first + 2) & 3
    barrier = pltpu.get_barrier_semaphore()

    def signal(sem, chip):
        pl.semaphore_signal(sem, inc=1, device_id=(chip,), device_id_type=pl.DeviceIdType.MESH)

    def remote(src, j, row, rows, chip, use, part):
        msg = ybuf.at[src, j, pl.ds(row, rows)]
        return pltpu.make_async_remote_copy(
            msg, msg,
            send_sems.at[(2 * use + part) * N_CHUNKS + j],
            recv_sems.at[(src + 2 * part) * N_CHUNKS + j],
            device_id=(chip,), device_id_type=pl.DeviceIdType.MESH)

    def chunk_msg(src, j, chip=0, use=0):
        return remote(src, j, 0, msg_rows(j), chip, use, 0)

    def part_msg(far_part, chip=0, use=0):
        j, part, row, rows, _ = far_part
        return remote(2, j, row, rows, chip, use, part)

    @pl.when(me != 2)
    def _():
        signal(barrier, right)
        signal(barrier, left)

    pl.when(me == 0)(lambda: signal(barrier, 2))

    o_ref[...] = jnp.zeros(o_ref.shape, f32)
    xs[:, :, pl.ds(SLOTS - 8, 8)] = jnp.zeros((E_LOC, 2, 8, 128), f32)

    @pl.when(me == 2)
    def _():
        pl.semaphore_wait(barrier, 3)
        signal(go_sem, 1)
        signal(go_sem, 3)

    pl.when(odd)(lambda: pl.semaphore_wait(barrier, 1))

    def fetch_rows(e, tok):
        tok = tok & (N_TOK - 1)
        for s in range(CAP):
            t = tok[s, 0]
            pltpu.make_async_copy(
                x_hbm.at[t >> 3, :, t & 7], xs.at[e, :, s], in_sems.at[N_CHUNKS + e]).start()

    def produce(j, rider):
        e, c, n = CHUNKS[j]
        if j == 0:
            w_copy(j).wait()
        if c == 0:
            rows = xs.at[e, :, pl.ds(0, CAP)]
            pltpu.make_async_copy(rows, rows, in_sems.at[N_CHUNKS + e]).wait()
        xe = jnp.concatenate([xs[e, 0], xs[e, 1]], axis=1).astype(bf16)
        filled = (tok_v[e] < N_TOK) & (iota((SLOTS, 128), 0) < CAP)
        if j > 0:
            w_copy(j).wait()
        w = [ws[e, :, t // 2, t % 2].reshape(D_IN, 128).astype(bf16) for t in range(c, c + 2 * n, 2)]
        if n == 2:
            y = [jnp.where(filled, jnp.dot(xe, t, preferred_element_type=f32), 0.0) for t in w]
            lo, hi = [pltpu.bitcast(v.astype(bf16).astype(f32), u32) for v in y]
            ybuf[me, j] = (lo >> 16) | hi
            return 0.0
        for h in range(2):
            half = slice(16 * h, 16 * h + 16)
            y = jnp.dot(xe[half], w[0], preferred_element_type=f32)
            y = jnp.where(filled[half], y, rider if h else 0.0)
            ybuf[me, j, pl.ds(8 * h, 8)] = pltpu.bitcast(y.astype(bf16), u32)
        if j not in LEADING:
            return 0.0
        return jnp.concatenate([jnp.zeros((8, 128), f32), pltpu.roll(y[8:], 1, 0)], axis=0)

    def send_early_far(j):
        mine = [p for p in FAR_PARTS if p[0] == j]
        for p in mine:
            (part_msg(p, 3, 1) if p[4] else part_msg(p, 0, 2)).start()
        if all(p[4] for p in mine):
            chunk_msg(2, j, 1, 0).start()

    def send_early_near(j):
        chunk_msg(me, j, first, 0).start()
        if j < 2:
            pl.when(me == 0)(chunk_msg(me, j, second, 1).start)
            return
        if j == 2:
            @pl.when(odd)
            def _():
                pl.semaphore_wait(go_sem, 1)
                for i in range(j):
                    chunk_msg(me, i, second, 1).start()
        chunk_msg(me, j, second, 1).start()

    def find_destinations():
        r = iota((4 * N_EXP, 128), 0)
        count = running_count(idx_v, r >> 2, r & 3)
        hits = jnp.concatenate([slot_hits(count[4 * g:4 * g + 4]) for g in range(N_EXP)], axis=0)
        tok = lax.dot_general(jnp.ones((16, 128), bf16), hits.astype(bf16), (((1,), (1,)), ((), ())),
                              preferred_element_type=f32)[:8]
        over = (iota(tok.shape, 1) & (SLOTS - 1)) >= CAP
        dropped = jnp.min(jnp.where(over, tok, N_TOK - 1.0), axis=1, keepdims=True)
        t = to_int(jnp.where(tok < N_TOK, tok, dropped)) & (N_TOK - 1)
        dest_v[...] = (((t >> 3) << 5) + (t & 7))[:1]
        dest_copy.start()

    def scatter(src, j, row=0, rows=None):
        e, c, n = CHUNKS[j]
        for r in range(row, row + (rows or msg_rows(j))):
            if n == 2:
                halves = ((r, c), (r, c + 2))
            elif 2 * r + 1 < CAP:
                halves = ((2 * r, c), (2 * r + 1, c))
            else:
                halves = ((2 * r, c), (2 * r, CHUNKS[j - 1][1]))
            word = ybuf[src, j, pl.ds(r, 1), :]
            start = {slot: dest_s[0, SLOTS * (E_LOC * src + e) + slot]
                     for slot in sorted({h[0] for h in halves})}
            for bits, (slot, tile) in zip((word << 16, word & jnp.uint32(0xFFFF0000)), halves):
                o_ref[pl.ds(start[slot] + 8 * tile, 1), :] = pltpu.bitcast(bits, f32)

    r = iota((4 * E_LOC, 128), 0)
    expert, block = E_LOC * me + (r >> 2), r & 3
    idx_copy.wait()
    count = running_count(idx_v, expert, block)
    count_v[...] = count
    tok = slot_tokens(count[:4])
    tok_v[0] = tok
    fetch_rows(0, tok)
    for e in range(1, E_LOC):
        tok_v[e] = slot_tokens(count_v[pl.ds(4 * e, 4), :])
    fetch_rows(1, tok_v[1])

    rider = 0.0
    for j in range(N_CHUNKS):
        rider = produce(j, rider)
        if j == 0:
            @pl.when(me == 0)
            def _():
                find_destinations()
                pl.semaphore_wait(barrier, 2)
        if j < N_EARLY:
            pl.when(me != 2)(functools.partial(send_early_near, j))
            pl.when(me == 2)(functools.partial(send_early_far, j))
        else:
            chunk_msg(me, j, jnp.where(me == 2, 0, first), 0).start()
            chunk_msg(me, j, second, 1).start()
        if j in (1, 2):
            fetch_rows(j + 1, tok_v[j + 1])

    @pl.when(me == 2)
    def _():
        for p in FAR_PARTS:
            j = p[0]
            if j >= N_EARLY:
                chunk_msg(2, j, 1, 2).start()
            elif not p[4]:
                part_msg(p, 3, 1).start()
                chunk_msg(2, j, 1, 0).start()

    @pl.when(me == 3)
    def _():
        for p in FAR_PARTS:
            if p[4]:
                part_msg(p).wait_recv()
                part_msg(p, 0, 2).start()

    @pl.when(odd)
    def _():
        for j in range(N_CHUNKS):
            chunk_msg(0, j).wait_recv()
            pl.when((me >> 1) == (j & 1))(chunk_msg(0, j, 2, 3).start)

    pl.when(me != 0)(find_destinations)
    dest_copy.wait()

    def scatter_chip(n, _):
        src = jnp.where(me == 2, (2 * n - 1) % 5,
                        jnp.where(n == 1, 0, jnp.where((n == 2) == (me == 1), 4 - me, 2)))
        src = jnp.where(n == 0, me, src)
        landed = (n == 0) | ((src == 0) & odd)
        relayed = (src == 2) & (me == 3)

        @pl.when(relayed)
        def _():
            for p in FAR_PARTS:
                if not p[4]:
                    part_msg(p).wait_recv()

        for batch in (range(6), range(6, N_CHUNKS)):
            @pl.when(jnp.logical_not(landed | relayed))
            def _():
                for j in batch:
                    chunk_msg(src, j).wait_recv()

            for j in batch:
                scatter(src, j)

    @pl.when(me != 0)
    def _():
        lax.fori_loop(0, N_DEV, scatter_chip, None)
        for j in range(N_CHUNKS):
            chunk_msg(me, j, first, 0).wait_send()

    @pl.when(me == 2)
    def _():
        for p in FAR_PARTS:
            part_msg(p, 3, 1).wait_send()
            if not p[4]:
                part_msg(p, 0, 2).wait_send()

    @pl.when(me == 3)
    def _():
        for p in FAR_PARTS:
            if p[4]:
                part_msg(p, 0, 2).wait_send()

    @pl.when(odd)
    def _():
        for j in range(N_CHUNKS):
            chunk_msg(me, j, second, 1).wait_send()
            pl.when((me >> 1) == (j & 1))(chunk_msg(0, j, 2, 3).wait_send)

    @pl.when(me == 0)
    def _():
        sent = [chunk_msg(0, j, 1, use) for j in range(N_CHUNKS) for use in (0, 1)]
        for src, k in ROOT_ORDER:
            if src is None:
                for _ in range(k):
                    sent.pop(0).wait_send()
            elif src == 0:
                scatter(0, k)
            elif src == 2:
                j, _, row, rows, _ = FAR_PARTS[k]
                part_msg(FAR_PARTS[k]).wait_recv()
                scatter(2, j, row, rows)
            else:
                chunk_msg(src, k).wait_recv()
                sent.append(chunk_msg(src, k, 4 - src, 2 + src // 2))
                sent[-1].start()
                scatter(src, k)
        assert not sent


def pallas_dist_moe_cap_ep_n512_d256_e4_h512_kernel(
    x: jax.Array,
    router_W: jax.Array,
    route_idx: jax.Array,
    expert_W: jax.Array,
):
    del router_W
    hbm = pl.BlockSpec(memory_space=pltpu.HBM)
    out = pl.pallas_call(
        moe_kernel,
        out_shape=jax.ShapeDtypeStruct((N_TOK * D_OUT // 128, 128), f32),
        in_specs=[hbm, hbm, hbm],
        out_specs=pl.BlockSpec(memory_space=pltpu.VMEM),
        scratch_shapes=[
            pltpu.VMEM((N_TOK // 128, 128), i32),
            pltpu.VMEM((4 * E_LOC, 128), f32),
            pltpu.VMEM((E_LOC, SLOTS, 128), i32),
            pltpu.VMEM((E_LOC, 2, SLOTS, 128), f32),
            pltpu.VMEM((E_LOC, D_IN // 8, 2, 2, 8, 128), f32),
            pltpu.VMEM((N_DEV, N_CHUNKS, SLOTS, 128), u32),
            pltpu.VMEM((1, N_EXP * SLOTS), i32),
            pltpu.SMEM((1, N_EXP * SLOTS), i32),
            pltpu.SemaphoreType.DMA((N_CHUNKS + E_LOC + 1,)),
            pltpu.SemaphoreType.DMA,
            pltpu.SemaphoreType.REGULAR,
            pltpu.SemaphoreType.DMA((8 * N_CHUNKS,)),
            pltpu.SemaphoreType.DMA(((N_DEV + 1) * N_CHUNKS,)),
        ],
        compiler_params=pltpu.CompilerParams(
            collective_id=0,
            disable_bounds_checks=True,
            disable_semaphore_checks=True,
            flags={"XLA_TPU_FORCE_LP_LLO_SCHEDULER": True},
        ),
    )(
        x.reshape(N_TOK // 8, 8, 2, 128).transpose(0, 2, 1, 3),
        route_idx.reshape(N_TOK // 128, 128),
        expert_W.reshape(E_LOC, D_IN // 8, 8, 2, 2, 128).transpose(0, 1, 3, 4, 2, 5),
    )
    return out.reshape(N_TOK // 8, 4, 8, 128).transpose(0, 2, 1, 3).reshape(N_TOK, D_OUT)
```

```python
import functools

import jax
import jax.numpy as jnp
from jax import lax
from jax.experimental import pallas as pl
from jax.experimental.pallas import tpu as pltpu

N_TOK, D_IN, D_OUT = 512, 256, 512
N_EXP, CAP, N_DEV = 16, 25, 4
E_LOC = N_EXP // N_DEV
SLOTS = 32
HALF = SLOTS // 2
f32, bf16, i32, u32 = jnp.float32, jnp.bfloat16, jnp.int32, jnp.uint32

CHUNKS = (
    (0, 0, 2), (0, 1, 2), (1, 0, 2), (1, 1, 2), (2, 0, 2),
    (2, 1, 1), (2, 3, 1), (3, 0, 1), (3, 1, 1), (3, 2, 1), (3, 3, 1),
)
LEADING = (5, 7, 9)
N_CHUNKS = len(CHUNKS)


def msg_rows(j):
    return CAP if CHUNKS[j][2] == 2 else CAP // 2 + (j not in LEADING)


N_EARLY = 5
FAR_PARTS = (
    (0, 0, 0, CAP, False), (1, 0, 0, CAP, True), (2, 0, 0, CAP, True), (3, 0, 0, CAP, True),
    (4, 0, 0, 7, False), (4, 1, 7, CAP - 7, True),
) + tuple((j, 0, 0, msg_rows(j), False) for j in range(N_EARLY, N_CHUNKS))

ROOT_ORDER = (
    (0, 0), (0, 1), (0, 2), (0, 3), (1, 0), (3, 0), (1, 1), (3, 1), (1, 2), (3, 2),
    (0, 4), (0, 5), (1, 3), (3, 3), (0, 6), (0, 7), (0, 8), (0, 9), (0, 10), (None, 22),
    (3, 4), (2, 0), (1, 4), (3, 5), (3, 6), (1, 5), (3, 7), (1, 6), (3, 8), (1, 7),
    (3, 9), (1, 8), (3, 10), (1, 9), (1, 10), (2, 1), (2, 4), (None, 14), (2, 6), (2, 2),
    (None, 8), (2, 7), (2, 8), (2, 3), (2, 9), (2, 10), (2, 5), (2, 11),
)


def iota(shape, dim):
    return lax.broadcasted_iota(i32, shape, dim)


def to_int(v):
    return pltpu.bitcast(v + 2.0**23, i32) & 0xFFFF


def running_count(idx_ref, expert, block):
    own = jnp.zeros(expert.shape, f32)
    before = jnp.zeros(expert.shape, f32)
    for k in range(N_TOK // 128):
        routed = jnp.broadcast_to(idx_ref[pl.ds(k, 1), :], expert.shape) & (N_EXP - 1)
        hit = routed == expert
        own = jnp.where(hit & (block == k), 1.0, own)
        if k < N_TOK // 128 - 1:
            before = before + jnp.where(hit & (block > k), 1.0, 0.0)
    upper = jnp.where(iota((128, 128), 0) <= iota((128, 128), 1), 1.0, 0.0).astype(bf16)
    ones = jnp.ones((128, 128), bf16)
    return (jnp.dot(own.astype(bf16), upper, preferred_element_type=f32)
            + jnp.dot(before.astype(bf16), ones, preferred_element_type=f32))


def slot_hits(count):
    slot = iota((SLOTS, 128), 0).astype(f32)
    hits = [jnp.where(jnp.broadcast_to(count[b:b + 1], slot.shape) <= slot, 1.0, 0.0)
            for b in range(N_TOK // 128)]
    return functools.reduce(jnp.add, hits)


def slot_tokens(count):
    hits = slot_hits(count)
    return to_int(jnp.broadcast_to(jnp.sum(hits, axis=1, keepdims=True), hits.shape))


def moe_kernel(x_hbm, idx_hbm, w_hbm, o_ref, idx_v, count_v, tok_v, xs, ws, ybuf, dest_v, dest_s,
               in_sems, dest_sem, go_sem, send_sems, recv_sems):
    idx_copy = pltpu.make_async_copy(idx_hbm, idx_v, in_sems.at[N_CHUNKS + E_LOC])
    dest_copy = pltpu.make_async_copy(dest_v, dest_s, dest_sem)

    def w_copy(j):
        e, c, n = CHUNKS[j]
        at = (e, slice(None), slice(None), c) if n == 2 else (e, slice(None), c // 2, c % 2)
        return pltpu.make_async_copy(w_hbm.at[at], ws.at[at], in_sems.at[j])

    idx_copy.start()
    for j in range(N_CHUNKS):
        w_copy(j).start(priority=1)

    me = lax.axis_index("i")
    right, left = (me + 1) & 3, (me + 3) & 3
    odd = (me & 1) == 1
    first = jnp.where(me == 3, right, left)
    second = (first + 2) & 3
    barrier = pltpu.get_barrier_semaphore()

    def signal(sem, chip):
        pl.semaphore_signal(sem, inc=1, device_id=(chip,), device_id_type=pl.DeviceIdType.MESH)

    def remote(src, j, row, rows, chip, use, part):
        msg = ybuf.at[src, j, pl.ds(row, rows)]
        return pltpu.make_async_remote_copy(
            msg, msg,
            send_sems.at[(2 * use + part) * N_CHUNKS + j],
            recv_sems.at[(src + 2 * part) * N_CHUNKS + j],
            device_id=(chip,), device_id_type=pl.DeviceIdType.MESH)

    def chunk_msg(src, j, chip=0, use=0):
        return remote(src, j, 0, msg_rows(j), chip, use, 0)

    def part_msg(far_part, chip=0, use=0):
        j, part, row, rows, _ = far_part
        return remote(2, j, row, rows, chip, use, part)

    @pl.when(me != 2)
    def _():
        signal(barrier, right)
        signal(barrier, left)

    pl.when(me == 0)(lambda: signal(barrier, 2))

    o_ref[...] = jnp.zeros(o_ref.shape, f32)
    xs[:, :, pl.ds(SLOTS - 8, 8)] = jnp.zeros((E_LOC, 2, 8, 128), f32)

    @pl.when(me == 2)
    def _():
        pl.semaphore_wait(barrier, 3)
        signal(go_sem, 1)
        signal(go_sem, 3)

    pl.when(odd)(lambda: pl.semaphore_wait(barrier, 1))

    def fetch_rows(e, tok):
        tok = tok & (N_TOK - 1)
        for s in range(CAP):
            t = tok[s, 0]
            sem = in_sems.at[N_CHUNKS + (E_LOC + 1 if e == 0 and s < HALF else e)]
            pltpu.make_async_copy(x_hbm.at[t >> 3, :, t & 7], xs.at[e, :, s], sem).start()

    def wait_rows(e, slot, slots, sem):
        rows = xs.at[e, :, pl.ds(slot, slots)]
        pltpu.make_async_copy(rows, rows, in_sems.at[N_CHUNKS + sem]).wait()

    def operands(e, slot, slots):
        at = pl.ds(slot, slots)
        xe = jnp.concatenate([xs[e, 0, at], xs[e, 1, at]], axis=1).astype(bf16)
        return xe, (tok_v[e, at] < N_TOK) & (iota((slots, 128), 0) < CAP - slot)

    def multiply(j, slot, xe, filled, rider=0.0):
        e, c, n = CHUNKS[j]
        y = []
        for t in range(c, c + 2 * n, 2):
            w = ws[e, :, t // 2, t % 2].reshape(D_IN, 128).astype(bf16)
            y.append(jnp.where(filled, jnp.dot(xe, w, preferred_element_type=f32), rider))
        if n == 2:
            lo, hi = [pltpu.bitcast(v.astype(bf16).astype(f32), u32) for v in y]
            ybuf[me, j, pl.ds(slot, xe.shape[0])] = (lo >> 16) | hi
        else:
            ybuf[me, j, pl.ds(slot // 2, xe.shape[0] // 2)] = pltpu.bitcast(y[0].astype(bf16), u32)
        return y[0]

    def send_early_far(j):
        mine = [p for p in FAR_PARTS if p[0] == j]
        for p in mine:
            (part_msg(p, 3, 1) if p[4] else part_msg(p, 0, 2)).start()
        if all(p[4] for p in mine):
            chunk_msg(2, j, 1, 0).start()

    def send_early_near(j):
        chunk_msg(me, j, first, 0).start()
        if j < 2:
            pl.when(me == 0)(chunk_msg(me, j, second, 1).start)
            return
        if j == 2:
            @pl.when(odd)
            def _():
                pl.semaphore_wait(go_sem, 1)
                for i in range(j):
                    chunk_msg(me, i, second, 1).start()
        chunk_msg(me, j, second, 1).start()

    def find_destinations():
        r = iota((4 * N_EXP, 128), 0)
        count = running_count(idx_v, r >> 2, r & 3)
        hits = jnp.concatenate([slot_hits(count[4 * g:4 * g + 4]) for g in range(N_EXP)], axis=0)
        tok = lax.dot_general(jnp.ones((16, 128), bf16), hits.astype(bf16), (((1,), (1,)), ((), ())),
                              preferred_element_type=f32)[:8]
        over = (iota(tok.shape, 1) & (SLOTS - 1)) >= CAP
        dropped = jnp.min(jnp.where(over, tok, N_TOK - 1.0), axis=1, keepdims=True)
        t = to_int(jnp.where(tok < N_TOK, tok, dropped)) & (N_TOK - 1)
        dest_v[...] = (((t >> 3) << 5) + (t & 7))[:1]
        dest_copy.start()

    def scatter(src, j, row=0, rows=None):
        e, c, n = CHUNKS[j]
        for r in range(row, row + (rows or msg_rows(j))):
            if n == 2:
                halves = ((r, c), (r, c + 2))
            elif 2 * r + 1 < CAP:
                halves = ((2 * r, c), (2 * r + 1, c))
            else:
                halves = ((2 * r, c), (2 * r, CHUNKS[j - 1][1]))
            word = ybuf[src, j, pl.ds(r, 1), :]
            start = {slot: dest_s[0, SLOTS * (E_LOC * src + e) + slot]
                     for slot in sorted({h[0] for h in halves})}
            for bits, (slot, tile) in zip((word << 16, word & jnp.uint32(0xFFFF0000)), halves):
                o_ref[pl.ds(start[slot] + 8 * tile, 1), :] = pltpu.bitcast(bits, f32)

    r = iota((4 * E_LOC, 128), 0)
    expert, block = E_LOC * me + (r >> 2), r & 3
    idx_copy.wait()
    count = running_count(idx_v, expert, block)
    count_v[...] = count
    tok = slot_tokens(count[:4])
    tok_v[0] = tok
    fetch_rows(0, tok)
    for e in range(1, E_LOC):
        tok_v[e] = slot_tokens(count_v[pl.ds(4 * e, 4), :])
    fetch_rows(1, tok_v[1])

    w_copy(0).wait()
    for slot, slots, sem in ((0, HALF, E_LOC + 1), (HALF, CAP - HALF, 0)):
        wait_rows(0, slot, slots, sem)
        multiply(0, slot, *operands(0, slot, HALF))
        pl.when(odd)(remote(me, 0, slot, slots, 0, 0, 0).start)

    @pl.when(me == 0)
    def _():
        find_destinations()
        pl.semaphore_wait(barrier, 2)
        chunk_msg(me, 0, first, 0).start()
        chunk_msg(me, 0, second, 1).start()

    pl.when(me == 2)(functools.partial(send_early_far, 0))

    rider = 0.0
    for j in range(1, N_CHUNKS):
        e, c, n = CHUNKS[j]
        if c == 0:
            wait_rows(e, 0, CAP, e)
        if n == 2:
            whole = operands(e, 0, SLOTS)
            w_copy(j).wait()
            multiply(j, 0, *whole)
        else:
            low, high = operands(e, 0, HALF), operands(e, HALF, HALF)
            w_copy(j).wait()
            multiply(j, 0, *low)
            y = multiply(j, HALF, *high, rider)
            rider = 0.0
            if j in LEADING:
                rider = jnp.concatenate([jnp.zeros((8, 128), f32), pltpu.roll(y[8:], 1, 0)], axis=0)
        if j < N_EARLY:
            pl.when(me != 2)(functools.partial(send_early_near, j))
            pl.when(me == 2)(functools.partial(send_early_far, j))
        else:
            chunk_msg(me, j, jnp.where(me == 2, 0, first), 0).start()
            chunk_msg(me, j, second, 1).start()
        if j in (1, 2):
            fetch_rows(j + 1, tok_v[j + 1])

    @pl.when(me == 2)
    def _():
        for p in FAR_PARTS:
            j = p[0]
            if j >= N_EARLY:
                chunk_msg(2, j, 1, 2).start()
            elif not p[4]:
                part_msg(p, 3, 1).start()
                chunk_msg(2, j, 1, 0).start()

    @pl.when(me == 3)
    def _():
        for p in FAR_PARTS:
            if p[4]:
                part_msg(p).wait_recv()
                part_msg(p, 0, 2).start()

    @pl.when(odd)
    def _():
        for j in range(N_CHUNKS):
            chunk_msg(0, j).wait_recv()
            pl.when((me >> 1) == (j & 1))(chunk_msg(0, j, 2, 3).start)

    pl.when(me != 0)(find_destinations)
    dest_copy.wait()

    def scatter_chip(n, _):
        src = jnp.where(me == 2, (2 * n - 1) % 5,
                        jnp.where(n == 1, 0, jnp.where((n == 2) == (me == 1), 4 - me, 2)))
        src = jnp.where(n == 0, me, src)
        landed = (n == 0) | ((src == 0) & odd)
        relayed = (src == 2) & (me == 3)

        @pl.when(relayed)
        def _():
            for p in FAR_PARTS:
                if not p[4]:
                    part_msg(p).wait_recv()

        for batch in (range(6), range(6, N_CHUNKS)):
            @pl.when(jnp.logical_not(landed | relayed))
            def _():
                for j in batch:
                    chunk_msg(src, j).wait_recv()

            for j in batch:
                scatter(src, j)

    @pl.when(me != 0)
    def _():
        lax.fori_loop(0, N_DEV, scatter_chip, None)
        for j in range(N_CHUNKS):
            chunk_msg(me, j, first, 0).wait_send()

    @pl.when(me == 2)
    def _():
        for p in FAR_PARTS:
            part_msg(p, 3, 1).wait_send()
            if not p[4]:
                part_msg(p, 0, 2).wait_send()

    @pl.when(me == 3)
    def _():
        for p in FAR_PARTS:
            if p[4]:
                part_msg(p, 0, 2).wait_send()

    @pl.when(odd)
    def _():
        for j in range(N_CHUNKS):
            chunk_msg(me, j, second, 1).wait_send()
            pl.when((me >> 1) == (j & 1))(chunk_msg(0, j, 2, 3).wait_send)

    @pl.when(me == 0)
    def _():
        sent = [chunk_msg(0, j, 1, use) for j in range(N_CHUNKS) for use in (0, 1)]
        for src, k in ROOT_ORDER:
            if src is None:
                for _ in range(k):
                    sent.pop(0).wait_send()
            elif src == 0:
                scatter(0, k)
            elif src == 2:
                j, _, row, rows, _ = FAR_PARTS[k]
                part_msg(FAR_PARTS[k]).wait_recv()
                scatter(2, j, row, rows)
            else:
                chunk_msg(src, k).wait_recv()
                sent.append(chunk_msg(src, k, 4 - src, 2 + src // 2))
                sent[-1].start()
                scatter(src, k)
        assert not sent


def pallas_dist_moe_cap_ep_n512_d256_e4_h512_kernel(
    x: jax.Array,
    router_W: jax.Array,
    route_idx: jax.Array,
    expert_W: jax.Array,
):
    del router_W
    hbm = pl.BlockSpec(memory_space=pltpu.HBM)
    out = pl.pallas_call(
        moe_kernel,
        out_shape=jax.ShapeDtypeStruct((N_TOK * D_OUT // 128, 128), f32),
        in_specs=[hbm, hbm, hbm],
        out_specs=pl.BlockSpec(memory_space=pltpu.VMEM),
        scratch_shapes=[
            pltpu.VMEM((N_TOK // 128, 128), i32),
            pltpu.VMEM((4 * E_LOC, 128), f32),
            pltpu.VMEM((E_LOC, SLOTS, 128), i32),
            pltpu.VMEM((E_LOC, 2, SLOTS, 128), f32),
            pltpu.VMEM((E_LOC, D_IN // 8, 2, 2, 8, 128), f32),
            pltpu.VMEM((N_DEV, N_CHUNKS, SLOTS, 128), u32),
            pltpu.VMEM((1, N_EXP * SLOTS), i32),
            pltpu.SMEM((1, N_EXP * SLOTS), i32),
            pltpu.SemaphoreType.DMA((N_CHUNKS + E_LOC + 2,)),
            pltpu.SemaphoreType.DMA,
            pltpu.SemaphoreType.REGULAR,
            pltpu.SemaphoreType.DMA((8 * N_CHUNKS,)),
            pltpu.SemaphoreType.DMA(((N_DEV + 1) * N_CHUNKS,)),
        ],
        compiler_params=pltpu.CompilerParams(
            collective_id=0,
            disable_bounds_checks=True,
            disable_semaphore_checks=True,
            flags={"XLA_TPU_FORCE_LP_LLO_SCHEDULER": True},
        ),
    )(
        x.reshape(N_TOK // 8, 8, 2, 128).transpose(0, 2, 1, 3),
        route_idx.reshape(N_TOK // 128, 128),
        expert_W.reshape(E_LOC, D_IN // 8, 8, 2, 2, 128).transpose(0, 1, 3, 4, 2, 5),
    )
    return out.reshape(N_TOK // 8, 4, 8, 128).transpose(0, 2, 1, 3).reshape(N_TOK, D_OUT)
```
